```python
import numpy as np

kernel_name = "dist_ring_attn_i_s256_d64"

def setup_inputs():
    S, D = 1024, 64
    q = np.random.randn(S, D).astype(np.float32)
    k = np.random.randn(S, D).astype(np.float32)
    v = np.random.randn(S, D).astype(np.float32)
    return {"q": q, "k": k, "v": v}

def reference(q: np.ndarray, k: np.ndarray, v: np.ndarray) -> np.ndarray:
    D = q.shape[1]
    scores = q @ k.T / np.sqrt(D)
    scores_max = np.max(scores, axis=1, keepdims=True)
    weights = np.exp(scores - scores_max)
    weights = weights / np.sum(weights, axis=1, keepdims=True)
    return weights @ v
```

```python
import jax
import jax.numpy as jnp
from jax import lax
from jax.experimental import pallas as pl
from jax.experimental.pallas import tpu as pltpu

N_DEV = 4


def pallas_dist_ring_attn_i_s256_d64_kernel(
    q: jax.Array,
    k: jax.Array,
    v: jax.Array,
):
    s_loc, d = q.shape
    scale = 1.0 / (d ** 0.5)

    def body(q_ref, k_ref, v_ref, o_ref, kv_ref, send_sems, recv_sems):
        my = lax.axis_index("i")

        barrier = pltpu.get_barrier_semaphore()
        for j in range(1, N_DEV):
            pl.semaphore_signal(
                barrier, inc=1,
                device_id=((my + j) % N_DEV,),
                device_id_type=pl.DeviceIdType.MESH,
            )

        kv_ref[my] = jnp.concatenate(
            [k_ref[...].astype(jnp.bfloat16), v_ref[...].astype(jnp.bfloat16)],
            axis=1,
        )

        pl.semaphore_wait(barrier, N_DEV - 1)

        sends = []
        for j in range(1, N_DEV):
            rdma = pltpu.make_async_remote_copy(
                src_ref=kv_ref.at[my],
                dst_ref=kv_ref.at[my],
                send_sem=send_sems.at[j],
                recv_sem=recv_sems.at[j],
                device_id=((my + j) % N_DEV,),
                device_id_type=pl.DeviceIdType.MESH,
            )
            rdma.start()
            sends.append(rdma)

        qp = jnp.concatenate(
            [(q_ref[...] * scale).astype(jnp.bfloat16),
             jnp.zeros((s_loc, d), jnp.bfloat16)],
            axis=1,
        )

        def block(src):
            kvb = kv_ref[src]
            s = lax.dot_general(
                qp, kvb, (((1,), (1,)), ((), ())),
                preferred_element_type=jnp.float32,
            )
            return s, kvb

        s, kvb = block(my)
        m = jnp.max(s, axis=1, keepdims=True)
        p = jnp.exp(s - m)
        l = jnp.sum(p, axis=1, keepdims=True)
        acc = jnp.dot(p.astype(jnp.bfloat16), kvb,
                      preferred_element_type=jnp.float32)

        for j in (1, 3, 2):
            src = (my - j) % N_DEV
            pltpu.make_async_remote_copy(
                src_ref=kv_ref.at[src],
                dst_ref=kv_ref.at[src],
                send_sem=send_sems.at[j],
                recv_sem=recv_sems.at[j],
                device_id=(src,),
                device_id_type=pl.DeviceIdType.MESH,
            ).wait_recv()
            s, kvb = block(src)
            m_new = jnp.maximum(m, jnp.max(s, axis=1, keepdims=True))
            alpha = jnp.exp(m - m_new)
            p = jnp.exp(s - m_new)
            l = alpha * l + jnp.sum(p, axis=1, keepdims=True)
            acc = alpha * acc + jnp.dot(p.astype(jnp.bfloat16), kvb,
                                        preferred_element_type=jnp.float32)
            m = m_new

        o_ref[...] = acc[:, d:] / l

        for rdma in sends:
            rdma.wait_send()

    return pl.pallas_call(
        body,
        out_shape=jax.ShapeDtypeStruct((s_loc, d), jnp.float32),
        in_specs=[pl.BlockSpec(memory_space=pltpu.VMEM)] * 3,
        out_specs=pl.BlockSpec(memory_space=pltpu.VMEM),
        scratch_shapes=[
            pltpu.VMEM((N_DEV, s_loc, 2 * d), jnp.bfloat16),
            pltpu.SemaphoreType.DMA((N_DEV,)),
            pltpu.SemaphoreType.DMA((N_DEV,)),
        ],
        compiler_params=pltpu.CompilerParams(collective_id=0),
    )(q, k, v)
```

```python
import jax
import jax.numpy as jnp
from jax import lax
from jax.experimental import pallas as pl
from jax.experimental.pallas import tpu as pltpu

N_DEV = 4
MESH = pl.DeviceIdType.MESH


def pallas_dist_ring_attn_i_s256_d64_kernel(q, k, v):
    s_loc, d = q.shape
    half = s_loc // 2
    scale = 1.0 / (d ** 0.5)

    def body(qt_hbm, kt_hbm, vt_hbm, ot_ref, qt_ref, kt_ref, vt_ref, kv_ref,
             loc_sems, send_sems, recv_sems, go_sem):
        my = lax.axis_index("i")
        barrier = pltpu.get_barrier_semaphore()

        ck = pltpu.make_async_copy(kt_hbm, kt_ref, loc_sems.at[0])
        cv = pltpu.make_async_copy(vt_hbm, vt_ref, loc_sems.at[1])
        cq = pltpu.make_async_copy(qt_hbm, qt_ref, loc_sems.at[2])

        def signal(sem, dev):
            pl.semaphore_signal(sem, inc=1, device_id=(dev,), device_id_type=MESH)

        def send(me, dst):
            return pltpu.make_async_remote_copy(
                src_ref=kv_ref.at[me], dst_ref=kv_ref.at[me],
                send_sem=send_sems.at[dst], recv_sem=recv_sems.at[me],
                device_id=(dst,), device_id_type=MESH)

        def recv_wait(src):
            pltpu.make_async_remote_copy(
                src_ref=kv_ref.at[src], dst_ref=kv_ref.at[src],
                send_sem=send_sems.at[src], recv_sem=recv_sems.at[src],
                device_id=(src,), device_id_type=MESH).wait_recv()

        def pack(me):
            ck.wait()
            kt = kt_ref[...]
            kstack = jnp.concatenate([kt[:, :half], kt[:, half:]], axis=0)
            kv_ref[me, 0:half, :] = kstack.T.astype(jnp.bfloat16)
            cv.wait()
            vt = vt_ref[...].astype(jnp.bfloat16)
            kv_ref[me, half:half + d, :] = vt[:, :half]
            kv_ref[me, half + d:, :] = vt[:, half:]

        def make_q():
            cq.wait()
            qs = (qt_ref[...] * scale).astype(jnp.bfloat16)
            z = jnp.zeros((d, s_loc), jnp.bfloat16)
            return (jnp.concatenate([qs, z], axis=0), jnp.concatenate([z, qs], axis=0))

        def attend(qq, src, state):
            q_lo, q_hi = qq
            kp = kv_ref[src, 0:half, :]
            s_lo = jnp.dot(kp, q_lo, preferred_element_type=jnp.float32)
            s_hi = jnp.dot(kp, q_hi, preferred_element_type=jnp.float32)
            m_blk = jnp.max(jnp.maximum(s_lo, s_hi), axis=0, keepdims=True)
            if state is None:
                m_new = m_blk
            else:
                m, l, acc = state
                m_new = jnp.maximum(m, m_blk)
            p_lo = jnp.exp(s_lo - m_new)
            p_hi = jnp.exp(s_hi - m_new)
            l_blk = jnp.sum(p_lo + p_hi, axis=0, keepdims=True)
            v_lo = kv_ref[src, half:half + d, :]
            v_hi = kv_ref[src, half + d:, :]
            o_blk = (jnp.dot(v_lo, p_lo.astype(jnp.bfloat16), preferred_element_type=jnp.float32)
                     + jnp.dot(v_hi, p_hi.astype(jnp.bfloat16), preferred_element_type=jnp.float32))
            if state is None:
                return m_new, l_blk, o_blk
            alpha = jnp.exp(m - m_new)
            return m_new, alpha * l + l_blk, alpha * acc + o_blk

        def finish(state, sends):
            m, l, acc = state
            ot_ref[...] = acc / l
            for s in sends:
                s.wait_send()

        R, A, L, B = 0, 1, 2, 3

        @pl.when(my == R)
        def _():
            signal(barrier, A)
            signal(barrier, B)
            ck.start(); cv.start(); cq.start()
            pack(R)
            pl.semaphore_wait(barrier, 2)
            sa = send(R, A); sa.start()
            sb = send(R, B); sb.start()
            qq = make_q()
            st = attend(qq, R, None)
            pl.semaphore_wait(go_sem, 1)
            sl = send(R, L); sl.start()
            for src in (A, B, L):
                recv_wait(src)
                st = attend(qq, src, st)
            finish(st, [sa, sb, sl])

        def side(me, other):
            signal(barrier, R)
            ck.start(); cv.start(); cq.start()
            pl.semaphore_wait(barrier, 1)
            signal(barrier, L)
            pack(me)
            sr = send(me, R); sr.start()
            qq = make_q()
            st = attend(qq, me, None)
            pl.semaphore_wait(go_sem, 1)
            sl = send(me, L); sl.start()
            so = send(me, other); so.start()
            for src in (R, L, other):
                recv_wait(src)
                st = attend(qq, src, st)
            finish(st, [sr, sl, so])

        @pl.when(my == A)
        def _():
            side(A, B)

        @pl.when(my == B)
        def _():
            side(B, A)

        @pl.when(my == L)
        def _():
            ck.start(); cv.start(); cq.start()
            pl.semaphore_wait(barrier, 2)
            for dev in (R, A, B):
                signal(go_sem, dev)
            pack(L)
            sr = send(L, R); sr.start()
            sa = send(L, A); sa.start()
            sb = send(L, B); sb.start()
            qq = make_q()
            st = attend(qq, L, None)
            for src in (A, B, R):
                recv_wait(src)
                st = attend(qq, src, st)
            finish(st, [sr, sa, sb])

    ot = pl.pallas_call(
        body,
        out_shape=jax.ShapeDtypeStruct((d, s_loc), jnp.float32),
        in_specs=[pl.BlockSpec(memory_space=pl.ANY)] * 3,
        out_specs=pl.BlockSpec(memory_space=pltpu.VMEM),
        scratch_shapes=[
            pltpu.VMEM((d, s_loc), jnp.float32),
            pltpu.VMEM((d, s_loc), jnp.float32),
            pltpu.VMEM((d, s_loc), jnp.float32),
            pltpu.VMEM((N_DEV, s_loc, 2 * d), jnp.bfloat16),
            pltpu.SemaphoreType.DMA((3,)),
            pltpu.SemaphoreType.DMA((N_DEV,)),
            pltpu.SemaphoreType.DMA((N_DEV,)),
            pltpu.SemaphoreType.REGULAR,
        ],
        compiler_params=pltpu.CompilerParams(collective_id=0),
    )(q.T, k.T, v.T)
    return ot.T
```

```python
import jax
import jax.numpy as jnp
from jax import lax
from jax.experimental import pallas as pl
from jax.experimental.pallas import tpu as pltpu

N_DEV = 4
MESH = pl.DeviceIdType.MESH
U = 32


def pallas_dist_ring_attn_i_s256_d64_kernel(q, k, v):
    s_loc, d = q.shape
    half = s_loc // 2
    scale = 1.0 / (d ** 0.5)
    bf = jnp.bfloat16
    f32 = jnp.float32

    R, A, L, B = 0, 1, 2, 3
    RT = {R: [(A, 0), (A, 4), (B, 0), (B, 4)] + [(L, u) for u in range(8)],
          A: [(R, 0), (B, 0), (B, 4), (L, 0), (L, 1), (L, 2), (L, 3), (L, 4)],
          B: [(R, 0), (A, 0), (A, 4), (L, 4), (L, 5), (L, 6), (L, 7), (L, 0)],
          L: [(A, 0), (B, 0), (R, 0), (R, 4)]}

    def body(qt_hbm, kt_hbm, vt_hbm, ot_ref, qt_ref, kt_ref, vt_ref, kv_ref,
             loc_sems, send_sem, recv_sems, go_sem):
        my = lax.axis_index("i")
        barrier = pltpu.get_barrier_semaphore()

        ck = pltpu.make_async_copy(kt_hbm, kt_ref, loc_sems.at[0])
        cv = pltpu.make_async_copy(vt_hbm, vt_ref, loc_sems.at[1])
        cq = pltpu.make_async_copy(qt_hbm, qt_ref, loc_sems.at[2])

        def signal(sem, dev):
            pl.semaphore_signal(sem, inc=1, device_id=(dev,), device_id_type=MESH)

        def desc(origin, u0, nu, dst):
            sl = pl.ds(u0 * U, nu * U)
            return pltpu.make_async_remote_copy(
                src_ref=kv_ref.at[origin, sl], dst_ref=kv_ref.at[origin, sl],
                send_sem=send_sem.at[0], recv_sem=recv_sems.at[RT[dst].index((origin, u0))],
                device_id=(dst,), device_id_type=MESH)

        class Comm:
            def __init__(self, me):
                self.n = 0
                self.me = me

            def send(self, origin, u0, nu, dst):
                desc(origin, u0, nu, dst).start()
                self.n += nu

            def recv(self, origin, u0, nu):
                desc(origin, u0, nu, self.me).wait_recv()

            def drain(self):
                assert self.n % 8 == 0
                blk = kv_ref.at[pl.ds(0, self.n // 8)]
                pltpu.make_async_remote_copy(
                    src_ref=blk, dst_ref=blk, send_sem=send_sem.at[0],
                    recv_sem=recv_sems.at[0], device_id=(self.me,),
                    device_id_type=MESH).wait_send()

        def pack_k(me):
            ck.wait()
            kt = kt_ref[...].astype(bf)
            for h in range(2):
                kv_ref[me, 2 * h * d:(2 * h + 1) * d, :] = kt[:, half * h:half * (h + 1)]

        def pack_v(me):
            cv.wait()
            vt = vt_ref[...].astype(bf)
            for h in range(2):
                kv_ref[me, (2 * h + 1) * d:(2 * h + 2) * d, :] = vt[:, half * h:half * (h + 1)]

        def make_q():
            cq.wait()
            return (qt_ref[...] * scale).astype(bf)

        def scores(qq, parts, state):
            ss = [lax.dot_general(kv_ref[src, 2 * h * d:(2 * h + 1) * d, :], qq,
                                  (((0,), (0,)), ((), ())), preferred_element_type=f32)
                  for src, h in parts]
            mx = ss[0]
            for s_ in ss[1:]:
                mx = jnp.maximum(mx, s_)
            m_new = jnp.max(mx, axis=0, keepdims=True)
            if state is not None:
                m_new = jnp.maximum(state[0], m_new)
            ps = [jnp.exp(s_ - m_new) for s_ in ss]
            sm = ps[0]
            for p_ in ps[1:]:
                sm = sm + p_
            l_blk = jnp.sum(sm, axis=0, keepdims=True)
            ps = [p_.astype(bf) for p_ in ps]
            if state is None:
                return m_new, l_blk, None, ps
            m, l, acc = state
            alpha = jnp.exp(m - m_new)
            return m_new, alpha * l + l_blk, alpha * acc, ps

        def attend(qq, parts, state):
            m, l, acc, ps = scores(qq, parts, state)
            for (src, h), p in zip(parts, ps):
                vh = kv_ref[src, (2 * h + 1) * d:(2 * h + 2) * d, :]
                o = jnp.dot(vh, p, preferred_element_type=f32)
                acc = o if acc is None else acc + o
            return m, l, acc

        def both(src):
            return [(src, 0), (src, 1)]

        def finish(state, cm):
            _, l, acc = state
            ot_ref[...] = acc / l
            cm.drain()

        @pl.when(my == R)
        def _():
            cm = Comm(R)
            signal(barrier, A)
            signal(barrier, B)
            ck.start(); cv.start(); cq.start()
            pack_k(R); pack_v(R)
            pl.semaphore_wait(barrier, 2)
            cm.send(R, 0, 8, A)
            cm.send(R, 0, 8, B)
            qq = make_q()
            st = attend(qq, both(R), None)
            cm.recv(B, 0, 4); cm.send(B, 0, 4, A)
            cm.recv(A, 0, 4); cm.send(A, 0, 4, B)
            st = attend(qq, [(B, 0), (A, 0)], st)
            cm.recv(B, 4, 4); cm.send(B, 4, 4, A)
            cm.recv(A, 4, 4); cm.send(A, 4, 4, B)
            st = attend(qq, [(B, 1), (A, 1)], st)
            for u in (0, 4, 1, 5):
                cm.recv(L, u, 1)
            _, l, acc, ps = scores(qq, both(L), st)
            inv = 1.0 / l
            acc = acc * inv
            pcat = jnp.concatenate(ps, axis=0)
            for u in (2, 6, 3, 7):
                cm.recv(L, u, 1)
            vcat = jnp.concatenate([kv_ref[L, d:2 * d, :], kv_ref[L, 3 * d:4 * d, :]], axis=1)
            o = jnp.dot(vcat, pcat, preferred_element_type=f32)
            ot_ref[...] = acc + o * inv
            cm.drain()

        def side(me, other, h):
            cm = Comm(me)
            signal(barrier, R)
            signal(barrier, L)
            ck.start(); cv.start(); cq.start()
            pl.semaphore_wait(barrier, 1)
            pack_k(me); pack_v(me)
            cm.send(me, 0, 4, R)
            cm.send(me, 4, 4, R)
            qq = make_q()
            st = attend(qq, both(me), None)
            pl.semaphore_wait(go_sem, 1)
            cm.send(me, 0, 8, L)
            for u in range(4 * h, 4 * h + 4):
                cm.recv(L, u, 1); cm.send(L, u, 1, R)
            cm.recv(R, 0, 8); cm.send(R, 4 * h, 4, L)
            st = attend(qq, both(R), st)
            cm.recv(L, 4 * (1 - h), 4)
            st = attend(qq, both(L), st)
            cm.recv(other, 0, 4)
            st = attend(qq, [(other, 0)], st)
            cm.recv(other, 4, 4)
            st = attend(qq, [(other, 1)], st)
            finish(st, cm)

        @pl.when(my == A)
        def _():
            side(A, B, 0)

        @pl.when(my == B)
        def _():
            side(B, A, 1)

        @pl.when(my == L)
        def _():
            cm = Comm(L)
            ck.start(); cv.start(); cq.start()
            pl.semaphore_wait(barrier, 2)
            signal(go_sem, A)
            signal(go_sem, B)
            pack_k(L)
            for u in (0, 1):
                cm.send(L, u, 1, A)
                cm.send(L, 4 + u, 1, B)
            pack_v(L)
            for u in (2, 3):
                cm.send(L, u, 1, A)
                cm.send(L, 4 + u, 1, B)
            cm.send(L, 4, 4, A)
            cm.send(L, 0, 4, B)
            qq = make_q()
            st = attend(qq, both(L), None)
            cm.recv(B, 0, 8)
            st = attend(qq, both(B), st)
            cm.recv(A, 0, 8)
            st = attend(qq, both(A), st)
            cm.recv(R, 0, 4)
            cm.recv(R, 4, 4)
            st = attend(qq, both(R), st)
            finish(st, cm)

    ot = pl.pallas_call(
        body,
        out_shape=jax.ShapeDtypeStruct((d, s_loc), jnp.float32),
        in_specs=[pl.BlockSpec(memory_space=pl.ANY)] * 3,
        out_specs=pl.BlockSpec(memory_space=pltpu.VMEM),
        scratch_shapes=[
            pltpu.VMEM((d, s_loc), jnp.float32),
            pltpu.VMEM((d, s_loc), jnp.float32),
            pltpu.VMEM((d, s_loc), jnp.float32),
            pltpu.VMEM((N_DEV, s_loc, 2 * d), jnp.bfloat16),
            pltpu.SemaphoreType.DMA((3,)),
            pltpu.SemaphoreType.DMA((1,)),
            pltpu.SemaphoreType.DMA((12,)),
            pltpu.SemaphoreType.REGULAR,
        ],
        compiler_params=pltpu.CompilerParams(collective_id=0),
    )(q.T, k.T, v.T)
    return ot.T
```
